```python
import numpy as np

kernel_name = "dist_mlp2_tp_i_m512_h1024_out512"

def setup_inputs():
    x = np.random.randn(512, 512).astype(np.float32)
    W1 = np.random.randn(512, 4096).astype(np.float32)
    W2 = np.random.randn(4096, 512).astype(np.float32)
    return {"x": x, "W1": W1, "W2": W2}

def reference(x: np.ndarray, W1: np.ndarray, W2: np.ndarray) -> np.ndarray:
    h = x @ W1
    h = np.maximum(h, 0.0)
    return h @ W2
```

```python
import jax
import jax.numpy as jnp
from jax import lax
from jax.experimental import pallas as pl
from jax.experimental.pallas import tpu as pltpu

_A, _MID, _D = 0, 1, 2
_HALF = 256
_TILE = 32
_LANES = 128
_HEAD = 8

_ROUTES = (
    "aa aa ed da",
    "aa aa aa da",
    "aa aa ed da",
    "aa aa ed ed",
    "dd da aa ed",
    "ea ed aa ed",
    "ed da da ed",
    "ed dd ed ed",
)

_LOADS = (
    """
    x02203 x12203 a3 x03303 x13303 a2 a0 x01103 x11103 a1 b3 b0 b1 x00000 x10000 b2
    x00013 x10013
    """,
    """
    x11103 a0 x10033 a1 a2 a3 b0 x13333 b1 b2 x01133 b3 x02203 x03322 x03300
    """,
    """
    x00002 x10002 a0 a1 a2 a3 b0 b1 b2 x03303 x13303 b3
    """,
)

_STEPS = (
    """
    ld22 x'20 x'21 x'22 h43 ld5 x'31 h73 x'23 x'30 h63 h72 x'32 h52 ld1 h62 x31 h60
    h53 h32 ld2 h70 h30 ld1 h40 x33 h42 h50 h33 h20 h23 h22 h31 ld2 h21 ld2 h61 ld1
    h41 ld2 h51 ld2 m43 ld4 m23 ld2 p43 m63 ld4 p23 h71 ld2 m73 ld1 p63 m53 ld4 m33
    ld1 p53 p33 p73 m20 ld6 m70 ld1 m40 ld2 p70 m60 ld4 m50 ld1 m30 ld2 p50 p40 m51
    ld4 m61 p60 m21 p51 h10 m41 m71 p61 p30 m22 m32 p20 p32 p22 h02 h03 m72 m62 h12
    p41 h00 h01 p72 p62 h11 h13 m13 p21 m02 p02 m42 p13 m52 p71 m31 m03 m10 p52 p31
    m00 p00 p03 f00 m11 m12 p12 f31 p42 p10 p11 f20 m01 p01 f50 f52 f10 f42 f30 f21
    f01 f61 f12 f41 f13 f62 f03 f23 f11
    """,
    """
    ld22 x'10 x'11 x'12 x'13 h'10 ld1 x'03 h'11 ld2 h'20 x'20 ld1 h'21 h'01 x'21 ld1
    h'00 x'22 h'12 h'31 h'22 h00 h'13 h'03 ld1 h'23 ld2 h'02 ld3 n'10 ld1 h'30 ld2
    x'23 n'20 ld3 m'10 ld2 m'20 h'33 ld1 g30 g50 h'32 ld4 g40 g20 m'00 ld2 m'30 ld1
    g00 g10 n'01 ld4 g70 h01 ld2 g60 m'01 ld3 m'21 ld1 g11 m'11 ld3 g41 g01 g51 m'31
    ld2 g31 n'12 ld2 n'22 ld1 h12 ld1 g71 h02 ld3 g21 g61 m'12 ld3 m'22 ld1 m'02 g52
    g32 g42 h03 g12 g02 g22 m'32 m00 h10 h11 a10 h13 g72 a00 m10 g62 m'23 a20 m'13
    g43 a30 m11 g33 g53 m'03 a21 m01 h22 a01 g23 h20 g13 a11 h21 h23 d30 a31 m20 g03
    m22 a40 d40 m21 d50 a52 m'33 m03 g73 a42 m12 d51 a51 m23 m02 d32 a41 h30 g63 a50
    h31 h32 d43 a32 h33 d02 a02 m13 d22 m30 a22 m31 d60 a60 m33 d41 a61 d61 m32 d73
    d20 d53 a43 d72 a62 a12 a53 d70 d63 a13 a23 a70 a03 a71 d71 d33 a33 d10 d42 a73
    d62 d21 d01 d12 d23 a72 d13 d52 d11 d00 d31 d03 a63
    """,
    """
    ld22 x'01 x'00 x00 x'02 ld1 h10 ld1 h00 x01 ld1 h01 h11 h20 ld1 x02 h30 h21 h31
    x10 h12 h02 h32 ld1 h22 x12 h33 x03 x11 h13 h23 ld1 h03 ld2 n30 ld3 n10 ld1 h50
    ld1 h40 ld2 n20 ld2 m10 ld2 m00 ld1 p10 m20 ld4 h51 ld1 p00 h41 ld3 p20 m30 ld2
    n21 ld1 h42 p30 n31 ld4 m21 ld1 m01 p21 m11 ld4 p01 m31 ld2 h43 p11 h52 ld4 p31
    m40 ld2 m41 h53 ld2 p40 n52 m52 m42 p52 m22 p42 m51 m50 p51 m32 p41 m12 h63 h61
    p50 m02 p32 h62 h60 p02 m60 p22 m61 m43 p60 h71 p61 m53 h73 m62 p43 m13 p62 p12
    h72 h70 m71 p53 m73 m23 p13 m03 p23 m70 m72 m63 p70 n33 m33 p03 p71 p33 p73 p72
    p63 f32 f22 f43 f51 f60 f40 f02 f53 f72 f73 f63 f71 f50 f33 f70
    """,
)


def _parse(role):
    steps = []
    for word in _STEPS[role].split():
        if word.startswith("ld"):
            steps.append(("ld", 0, int(word[2:]), 0))
        else:
            steps.append((word[0], int("'" in word), int(word[-2]), int(word[-1])))
    return steps


def _passes_on(role, j, c):
    return _ROUTES[j].split()[c][1] == "a.d"[role]


def _num_sends(role):
    n = sum(
        op in "xpgad" or (op == "f" and _passes_on(role, j, c))
        for op, _, j, c in _parse(role)
    )
    return n if role == _MID else 2 * n


def _result_order(role):
    if role != _MID:
        return [(j, c) for op, _, j, c in _parse(_MID) if op == "a.d"[role]]
    queue = []
    for end in (_A, _D):
        sent = [
            (j, c) for op, _, j, c in _parse(end) if op == "f" and _passes_on(end, j, c)
        ]
        queue += [(i - len(sent), tile) for i, tile in enumerate(sent)]
    return [tile for _, tile in sorted(queue)]


_RECV_GROUPS = 5


class _Chip:
    def __init__(self, role, flip, barrier, refs):
        self.role = role
        self.flip = flip
        self.barrier = barrier
        (
            self.x_hbm, self.w1_hbm, self.w2_hbm, self.out,
            self.x_f32, self.w1, self.w2, self.x, self.hidden, self.hidden_acc,
            self.partial, self.outbox, self.inbox,
            self.load_sems, self.recv_sems, self.send_sems,
        ) = refs
        self.steps = _parse(role)
        self.arrived = set()
        self.num_sent = 0
        self.sending = []
        self.terms = {}
        self.fresh = {}
        self.fresh_hidden = None
        self.to_start = []
        self.x_read = {}
        for i, name in enumerate(_LOADS[role].split()):
            index = [int(digit) for digit in name[1:]]
            if name[0] == "a":
                self.to_start.append((("w1", *index), index))
            elif name[0] == "b":
                self.to_start += [
                    (("w2", *index, piece // 8), (*index, piece)) for piece in range(16)
                ]
            else:
                what = ("x", 12 + i, *index)
                self.to_start.append((what, what[1:]))
                half, j0, j1, k0, k1 = index
                for j in range(j0, j1 + 1):
                    for k in range(k0, k1 + 1):
                        self.x_read[half, j, k] = what

    @staticmethod
    def rows(half, j, n=1):
        return pl.ds(_HALF * half + _TILE * j, _TILE * n)

    def global_rows(self, half, j, n=1):
        if self.role != _MID:
            return self.rows(half, j, n)
        start = _HALF * (half ^ self.flip) + _TILE * j
        return pl.ds(pl.multiple_of(start, _TILE), _TILE * n)

    @staticmethod
    def lanes(c, n=1):
        return pl.ds(_LANES * c, _LANES * n)

    def out_tile(self, half, j, c):
        return self.out.at[self.global_rows(half, j), self.lanes(c)]

    def read(self, kind, *index):
        if kind == "w1":
            (k,) = index
            block = self.lanes(k) if k else pl.ds(_HEAD, _LANES - _HEAD)
            src, dst, sem = self.w1_hbm.at[block], self.w1.at[block], k
        elif kind == "w2":
            c, piece = index
            where = pl.ds(8 * (piece // 4), 8), pl.ds(8 * (piece % 4), 8)
            src = self.w2_hbm.at[(*where, self.lanes(c))]
            dst, sem = self.w2.at[(c, *where)], 4 + 2 * c + piece // 8
        else:
            sem, half, j0, j1, k0, k1 = index
            rows, lanes = (half, 2 * j0, 2 * (j1 - j0 + 1)), self.lanes(k0, k1 - k0 + 1)
            src = self.x_hbm.at[self.global_rows(*rows), lanes]
            dst = self.x_f32.at[self.rows(*rows), lanes]
        return pltpu.make_async_copy(src, dst, self.load_sems.at[sem])

    def start_reads(self, n):
        for _ in range(n):
            what, index = self.to_start.pop(0)
            self.read(what[0], *index).start()

    def wait_read(self, what):
        if what in self.arrived:
            return
        self.arrived.add(what)
        assert all(what != other for other, _ in self.to_start), what
        if what[0] == "x":
            self.read(*what).wait()
            half, j0, j1, k0, k1 = what[2:]
            rows = self.rows(half, 2 * j0, 2 * (j1 - j0 + 1))
            for k in range(k0, k1 + 1):
                self.x[k, rows] = self.x_f32[rows, self.lanes(k)].astype(jnp.bfloat16)
            return
        if what[0] == "w1":
            block, sem = self.w1.at[self.lanes(what[1])], what[1]
        else:
            _, c, part = what
            block, sem = self.w2.at[c, pl.ds(16 * part, 16)], 4 + 2 * c + part
        pltpu.make_async_copy(block, block, self.load_sems.at[sem]).wait()

    def message(self, src, dst, group, j, c, chip, send_sem):
        return pltpu.make_async_remote_copy(
            src_ref=src,
            dst_ref=dst,
            send_sem=self.send_sems.at[send_sem],
            recv_sem=self.recv_sems.at[32 * group + 4 * j + c],
            device_id=(chip,),
            device_id_type=pl.DeviceIdType.MESH,
        )

    def send(self, src, dst, group, j, c, chip):
        if self.num_sent == 0:
            pl.semaphore_wait(self.barrier, 2)
        copy = self.message(src, dst, group, j, c, chip, self.num_sent)
        copy.start()
        self.num_sent += 1
        self.sending.append(copy)

    def retire_sends(self, keep):
        while len(self.sending) > keep:
            self.sending.pop(0).wait_send()

    def receive(self, dst, group, j, c):
        if (group, j, c) not in self.arrived:
            self.arrived.add((group, j, c))
            neighbour = 0 if self.role == _MID else 1
            self.message(dst, dst, group, j, c, neighbour, 0).wait_recv()

    def need_x(self, half, j, k):
        if (half, j, k) in self.x_read:
            self.wait_read(self.x_read[half, j, k])
        else:
            self.receive(self.x.at[k, self.rows(half, 2 * j, 2)], 4, 4 * half + j, k)

    def received(self, slot, half, j, c):
        return self.inbox[slot, c, self.rows(half, j)].astype(jnp.float32)

    def own(self, half, j, c):
        if (half, j, c) in self.fresh:
            return self.fresh.pop((half, j, c))
        return self.partial[c, self.rows(half, j)]

    def matmul(self, i, lhs, rhs):
        result = jnp.dot(
            jnp.concatenate(lhs, axis=0),
            rhs.astype(jnp.bfloat16),
            preferred_element_type=jnp.float32,
        )
        self.store_hidden()
        used_next = set()
        for op, _, j, c in self.steps[i + 1 :]:
            if op in "hmn":
                break
            halves = {"p": (0, 1), "g": (1,), "a": (0,), "d": (0,)}.get(op, ())
            used_next.update((half, j, c) for half in halves)
        for half, j, c in [tile for tile in self.fresh if tile not in used_next]:
            self.partial[c, self.rows(half, j)] = self.fresh.pop((half, j, c))
        return [result[:_TILE], result[_TILE:]]

    def store_hidden(self):
        if self.fresh_hidden is None:
            return
        tiles, values, term = self.fresh_hidden
        self.fresh_hidden = None
        for tile, value in zip(tiles, values):
            rows = self.rows(*tile)
            if term > 0:
                value += self.hidden_acc[rows]
            if term < 3:
                self.hidden_acc[rows] = value
            else:
                self.hidden[rows] = jnp.maximum(value, 0.0).astype(jnp.bfloat16)

    def first_layer(self, i, tiles, k):
        for half, j in tiles:
            self.need_x(half, j // 2, k)
        self.wait_read(("w1", k))
        lhs = [self.x[k, self.rows(*tile)] for tile in tiles]
        values = self.matmul(i, lhs, self.w1[self.lanes(k)])
        term = self.terms.get(tiles, 0)
        self.terms[tiles] = term + 1
        self.fresh_hidden = tiles, values, term
        if next(op for op, *_ in self.steps[i + 1 :] if op != "ld") in "hmn":
            self.store_hidden()

    def second_layer(self, i, tiles, c, stop):
        assert self.terms[tiles] == 4, tiles
        start = self.terms.get((tiles, c), 0)
        self.terms[tiles, c] = stop
        for part in range(start, stop):
            self.wait_read(("w2", c, part))
        if self.fresh_hidden and self.fresh_hidden[0] == tiles:
            self.store_hidden()
        lhs = [self.hidden[self.rows(*t), 512 * start : 512 * stop] for t in tiles]
        rhs = self.w2[c, 16 * start : 16 * stop].reshape(-1, _LANES)
        for tile, value in zip(tiles, self.matmul(i, lhs, rhs)):
            self.fresh[(*tile, c)] = value + self.own(*tile, c) if start else value

    def end_step(self, op, j, c):
        route = _ROUTES[j].split()[c][0]
        rows = [self.rows(half, j) for half in (0, 1)]
        if op == "p":
            relay = (route == "a") == (self.role == _A)
            for half in (0, 1) if relay else ():
                self.receive(self.inbox.at[0, c, rows[half]], half, j, c)
            for half in (0, 1):
                value = self.own(half, j, c)
                if relay:
                    value += self.received(0, half, j, c)
                self.outbox[c, rows[half]] = value.astype(jnp.bfloat16)
            slot = self.role // 2
            for half in (0, 1):
                src, dst = self.outbox.at[c, rows[half]], self.inbox.at[slot, c, rows[0]]
                self.send(src, dst, slot, j, c, 1 + 2 * half)
            return
        self.retire_sends(max(24, len(self.sending) - 10))
        self.complete(j, c)
        for half in (0, 1) if _passes_on(self.role, j, c) else ():
            tile = self.out_tile(half, j, c)
            self.send(tile, tile, 2, j, c, 3 - 2 * half)

    def complete(self, j, c):
        if (2, j, c) in self.arrived:
            return
        if self.role == _MID:
            self.receive(self.out_tile(1, j, c), 2, j, c)
        elif _ROUTES[j].split()[c][0] == "a.e"[self.role]:
            for half in (0, 1):
                self.receive(self.inbox.at[1, c, self.rows(half, j)], 2 + half, j, c)
            for half in (0, 1):
                mine = self.outbox[c, self.rows(half, j)].astype(jnp.float32)
                total = mine + self.received(1, half, j, c)
                self.out[self.rows(half, j), self.lanes(c)] = total.astype(jnp.bfloat16)
        else:
            for half in (0, 1):
                self.receive(self.out_tile(half, j, c), 2 + half, j, c)

    def middle_step(self, op, j, c):
        route = _ROUTES[j].split()[c][0]
        if op == "g":
            self.outbox[c, self.rows(1, j)] = self.own(1, j, c).astype(jnp.bfloat16)
            src = self.outbox.at[c, self.rows(1, j)]
            dst = self.inbox.at[0, c, self.global_rows(1, j)]
            self.send(src, dst, 1 - self.flip, j, c, _A if route == "a" else _D)
            return
        rows = self.rows(0, j)
        other = int(op == "a")
        src = dst = self.out_tile(0, j, c)
        if route == "d":
            if op == "a":
                for slot in (0, 1):
                    self.receive(self.inbox.at[slot, c, rows], slot, j, c)
                total = self.own(0, j, c) + self.received(0, 0, j, c)
                total += self.received(1, 0, j, c)
                self.out[self.global_rows(0, j), self.lanes(c)] = total.astype(jnp.bfloat16)
        else:
            self.receive(self.inbox.at[other, c, rows], other, j, c)
            if (route == "a") == (op == "a"):
                pair = self.own(0, j, c) + self.received(other, 0, j, c)
                self.outbox[c, rows] = pair.astype(jnp.bfloat16)
                src = self.outbox.at[c, rows]
                dst = self.inbox.at[1, c, self.global_rows(0, j)]
            else:
                total = self.outbox[c, rows].astype(jnp.float32)
                total += self.received(other, 0, j, c)
                self.out[self.global_rows(0, j), self.lanes(c)] = total.astype(jnp.bfloat16)
        self.send(src, dst, 2 + self.flip, j, c, _A if op == "a" else _D)

    def pass_x(self, half, j, k):
        block = self.rows(half, 2 * j, 2)
        if self.role == _MID:
            self.need_x(half, j, k)
            dst = self.x.at[k, self.global_rows(half, 2 * j, 2)]
            self.send(self.x.at[k, block], dst, 4, 4 * (half ^ self.flip) + j, k, _D)
            return
        for flip in (0, 1):
            self.need_x(flip, j, k)
        for flip in (0, 1):
            src = self.x.at[k, self.rows(half ^ flip, 2 * j, 2)]
            self.send(src, self.x.at[k, block], 4, 4 * half + j, k, 1 + 2 * flip)

    def first_step(self):
        self.start_reads(self.steps[0][2])

    def other_steps(self):
        del self.to_start[: self.steps[0][2]]
        for i, (op, half, j, c) in list(enumerate(self.steps))[1:]:
            if self.role == _MID:
                tiles = ((half, 2 * j), (half, 2 * j + 1))
            else:
                tiles = ((0, j), (1, j))
            if op == "ld":
                self.start_reads(j)
            elif op == "x":
                self.pass_x(half, j, c)
            elif op == "h":
                self.first_layer(i, tiles, c)
            elif op in "mn":
                self.second_layer(i, tiles, c, 2 if op == "m" else 1)
            elif self.role == _MID:
                self.middle_step(op, j, c)
            else:
                self.end_step(op, j, c)
        results = _result_order(self.role)
        self.retire_sends(8)
        for tile in results[:-2]:
            self.complete(*tile)
        self.retire_sends(0)
        for tile in results[-2:]:
            self.complete(*tile)


def _kernel(*refs):
    w1_hbm, w1, load_sems = refs[1], refs[5], refs[-3]
    head = pl.ds(0, _HEAD)
    pltpu.make_async_copy(w1_hbm.at[head], w1.at[head], load_sems.at[0]).start()

    position = lax.axis_index("i")
    barrier = pltpu.get_barrier_semaphore()
    for neighbour in (position ^ 1, position ^ 3):
        pl.semaphore_signal(
            barrier, inc=1, device_id=(neighbour,), device_id_type=pl.DeviceIdType.MESH
        )

    flip = position >> 1
    is_role = [position == _A, (position & 1) == 1, position == _D]

    def on_role(role, steps):
        pl.when(is_role[role])(lambda: steps(_Chip(role, flip, barrier, refs)))

    for role in (_D, _MID, _A):
        on_role(role, _Chip.first_step)
    for role in (_A, _D, _MID):
        on_role(role, _Chip.other_steps)


def pallas_dist_mlp2_tp_i_m512_h1024_out512_kernel(
    x: jax.Array,
    W1: jax.Array,
    W2: jax.Array,
):
    f32, bf16 = jnp.float32, jnp.bfloat16
    params = {}
    if jax.__version_info__ >= (0, 12):
        params = dict(
            flags={"XLA_TPU_RESCHEDULE_DMA_DONES": True},
            disable_semaphore_checks=True,
        )
    return pl.pallas_call(
        _kernel,
        out_shape=jax.ShapeDtypeStruct((512, 512), bf16),
        in_specs=[pl.BlockSpec(memory_space=pl.ANY)] * 3,
        out_specs=pl.BlockSpec(memory_space=pltpu.VMEM),
        scratch_shapes=[
            pltpu.VMEM((512, 512), f32),
            pltpu.VMEM((512, 1024), f32),
            pltpu.VMEM((4, 32, 32, _LANES), f32),
            pltpu.VMEM((4, 512, _LANES), bf16),
            pltpu.VMEM((512, 1024), bf16),
            pltpu.VMEM((512, 1024), f32),
            pltpu.VMEM((4, 512, _LANES), f32),
            pltpu.VMEM((4, 512, _LANES), bf16),
            pltpu.VMEM((2, 4, 512, _LANES), bf16),
            pltpu.SemaphoreType.DMA((12 + max(len(s.split()) for s in _LOADS),)),
            pltpu.SemaphoreType.DMA((32 * _RECV_GROUPS,)),
            pltpu.SemaphoreType.DMA((max(map(_num_sends, (_A, _MID, _D))),)),
        ],
        compiler_params=pltpu.CompilerParams(collective_id=0, **params),
    )(x, W1, W2.reshape(32, 32, 512))
```
